```python
import numpy as np

kernel_name = "dist_sum_ax0_xy_m2048_n1024"

def setup_inputs():
    return {"x": np.random.randn(4096, 2048).astype(np.float32)}

def reference(x: np.ndarray) -> np.ndarray:
    return np.sum(x, axis=0, keepdims=True)
```

```python
import jax
import jax.numpy as jnp
from jax import lax
from jax.experimental import pallas as pl
from jax.experimental.pallas import tpu as pltpu

_MESH = pl.DeviceIdType.MESH

_RAW = 96
_CHUNKS = (1808, 112)
_TAIL = 32
_NCOL = 4


def _colsum8(ref, r0, nr, c0, nc, acc, blk=256):
    r, end = r0, r0 + nr
    while r < end:
        b = min(blk, end - r)
        v = ref[pl.ds(r, b), pl.ds(c0, nc)].reshape(b // 8, 8, nc).sum(0)
        acc = v if acc is None else acc + v
        r += b
    return acc


def pallas_dist_sum_ax0_xy_m2048_n1024_kernel(
x: jax.Array,
):
    m, n = x.shape
    assert _RAW + sum(_CHUNKS) + _TAIL == m
    w = n // _NCOL

    def body(x_hbm, o_ref, buf, rawbuf, sbuf, rbuf, csem, tsem, ssem, rsem, rawsem):
        chunk_cps = []
        r0 = 0
        for c, nr in enumerate(_CHUNKS):
            cp = pltpu.make_async_copy(
                x_hbm.at[pl.ds(_RAW + r0, nr)], buf.at[pl.ds(r0, nr)], csem.at[c])
            cp.start()
            chunk_cps.append((cp, r0, nr))
            r0 += nr
        tail_cps = []
        for c in range(_NCOL):
            cp = pltpu.make_async_copy(
                x_hbm.at[pl.ds(_RAW + r0, _TAIL), pl.ds(c * w, w)],
                buf.at[pl.ds(r0, _TAIL), pl.ds(c * w, w)], tsem.at[c])
            cp.start()
            tail_cps.append(cp)

        peer = (1 - lax.axis_index("x"), lax.axis_index("y"))
        barrier = pltpu.get_barrier_semaphore()
        pl.semaphore_signal(barrier, 1, device_id=peer, device_id_type=_MESH)
        pl.semaphore_wait(barrier, 1)

        raw = pltpu.make_async_remote_copy(
            x_hbm.at[pl.ds(0, _RAW)], rawbuf, rawsem.at[0], rawsem.at[1],
            device_id=peer, device_id_type=_MESH)
        raw.start()
        raw.wait_recv()
        acc = _colsum8(rawbuf, 0, _RAW, 0, n, None)
        raw.wait_send()

        for cp, rr, nr in chunk_cps:
            cp.wait()
            acc = _colsum8(buf, rr, nr, 0, n, acc)

        exs = []
        for c in range(_NCOL):
            tail_cps[c].wait()
            a = _colsum8(buf, r0, _TAIL, c * w, w, acc[:, c * w:(c + 1) * w])
            sbuf[c] = a.sum(0, keepdims=True)
            ex = pltpu.make_async_remote_copy(
                sbuf.at[c], rbuf.at[c], ssem.at[c], rsem.at[c],
                device_id=peer, device_id_type=_MESH)
            ex.start()
            exs.append(ex)
        for ex in exs:
            ex.wait_send()
        for c, ex in enumerate(exs):
            ex.wait_recv()
            o_ref[:, pl.ds(c * w, w)] = sbuf[c] + rbuf[c]

    return pl.pallas_call(
        body,
        out_shape=jax.ShapeDtypeStruct((1, n), x.dtype),
        in_specs=[pl.BlockSpec(memory_space=pl.ANY)],
        out_specs=pl.BlockSpec(memory_space=pltpu.VMEM),
        scratch_shapes=[
            pltpu.VMEM((m - _RAW, n), jnp.float32),
            pltpu.VMEM((_RAW, n), jnp.float32),
            pltpu.VMEM((_NCOL, 1, w), jnp.float32),
            pltpu.VMEM((_NCOL, 1, w), jnp.float32),
            pltpu.SemaphoreType.DMA((len(_CHUNKS),)),
            pltpu.SemaphoreType.DMA((_NCOL,)),
            pltpu.SemaphoreType.DMA((_NCOL,)),
            pltpu.SemaphoreType.DMA((_NCOL,)),
            pltpu.SemaphoreType.DMA((2,)),
        ],
        compiler_params=pltpu.CompilerParams(
            collective_id=0,
            disable_bounds_checks=True,
            disable_semaphore_checks=True,
        ),
    )(x)
```

```python
import jax
import jax.numpy as jnp
from jax import lax
from jax.experimental import pallas as pl
from jax.experimental.pallas import tpu as pltpu

_MESH = pl.DeviceIdType.MESH

_RX = 112
_RY = 72
_MIDS = (96, 32)
_TAIL = 48
_LANES = 128


def _colsum8(ref, r0, nr, acc, blk=256):
    n = ref.shape[-1]
    r, end = r0, r0 + nr
    while r < end:
        b = min(blk, end - r)
        v = ref[pl.ds(r, b), :].reshape(b // 8, 8, n).sum(0)
        acc = v if acc is None else acc + v
        r += b
    return acc


def _sum_tiles(vals):
    a, b = vals[0], vals[1]
    for i, v in enumerate(vals[2:]):
        if i % 2 == 0:
            a = a + v
        else:
            b = b + v
    v = a + b
    v = v + pltpu.roll(v, 4, 0)
    v = (v + pltpu.roll(v, 1, 0)) + (pltpu.roll(v, 2, 0) + pltpu.roll(v, 3, 0))
    return v[0:1, :]


def pallas_dist_sum_ax0_xy_m2048_n1024_kernel(
x: jax.Array,
):
    m, n = x.shape
    first = _RX + _RY
    chunks = (m - first - sum(_MIDS) - _TAIL,) + _MIDS
    tail0 = m - _TAIL
    ncol = n // _LANES

    def body(x_hbm, o_ref, buf, xraw, yraw, ysend, yres, sbuf, rbuf,
             csem, tsem, ssem, rsem, xsem, ysem, yready):
        chunk_cps = []
        r0 = first
        for c, nr in enumerate(chunks):
            rows = pl.ds(r0, nr)
            cp = pltpu.make_async_copy(x_hbm.at[rows], buf.at[rows], csem.at[c])
            cp.start()
            chunk_cps.append((cp, r0, nr))
            r0 += nr
        tail_cps = []
        for c in range(ncol):
            blk = (pl.ds(tail0, _TAIL), pl.ds(c * _LANES, _LANES))
            cp = pltpu.make_async_copy(x_hbm.at[blk], buf.at[blk], tsem.at[c])
            cp.start()
            tail_cps.append(cp)

        mx = lax.axis_index("x")
        my = lax.axis_index("y")
        px = (1 - mx, my)
        py = (mx, 1 - my)

        x_own = pltpu.make_async_copy(
            x_hbm.at[pl.ds(0, _RX)], buf.at[pl.ds(0, _RX)], xsem.at[2])
        x_raw = pltpu.make_async_remote_copy(
            x_hbm.at[pl.ds(0, _RX)], xraw, xsem.at[0], xsem.at[1],
            device_id=px, device_id_type=_MESH)
        y_raw = pltpu.make_async_remote_copy(
            x_hbm.at[pl.ds(_RX, _RY)], yraw, ysem.at[0], ysem.at[1],
            device_id=py, device_id_type=_MESH)
        y_back = pltpu.make_async_remote_copy(
            ysend, yres, ysem.at[2], ysem.at[3],
            device_id=py, device_id_type=_MESH)

        barrier = pltpu.get_barrier_semaphore()
        pl.semaphore_signal(barrier, 1, device_id=px, device_id_type=_MESH)

        @pl.when(mx == 0)
        def _():
            x_own.start()

        @pl.when(my == 0)
        def _():
            pl.semaphore_signal(barrier, 1, device_id=py, device_id_type=_MESH)
            pl.semaphore_wait(barrier, 1)

        @pl.when(my == 1)
        def _():
            pl.semaphore_wait(barrier, 2)
            pl.semaphore_signal(yready, 1, device_id=py, device_id_type=_MESH)

        @pl.when(mx == 1)
        def _():
            x_raw.start()

        @pl.when(my == 0)
        def _():
            pl.semaphore_wait(yready, 1)

        y_raw.start()

        y_raw.wait_recv()
        ysend[...] = _colsum8(yraw, 0, _RY, None).sum(0, keepdims=True)
        y_back.start()

        cp, r0, nr = chunk_cps[0]
        cp.wait()
        acc = _colsum8(buf, r0, nr, None)

        def add_x_rows(acc):
            x_own.wait()
            acc = _colsum8(buf, 0, _RX, acc)
            x_raw.wait_recv()
            return _colsum8(xraw, 0, _RX, acc)

        acc = lax.cond(mx == 0, add_x_rows, lambda acc: acc, acc)

        y_back.wait_recv()
        row = lax.broadcasted_iota(jnp.int32, (8, n), 0)
        acc = acc + jnp.where(row == 0, jnp.broadcast_to(yres[...], (8, n)), 0.0)

        for cp, r0, nr in chunk_cps[1:]:
            cp.wait()
            acc = _colsum8(buf, r0, nr, acc)

        parts = []
        for c in range(ncol):
            cols = pl.ds(c * _LANES, _LANES)
            tail_cps[c].wait()
            sbuf[:, cols] = _sum_tiles(
                [acc[:, c * _LANES:(c + 1) * _LANES]]
                + [buf[pl.ds(tail0 + 8 * i, 8), cols] for i in range(_TAIL // 8)])
            part = pltpu.make_async_remote_copy(
                sbuf.at[:, cols], rbuf.at[:, cols], ssem.at[c], rsem.at[c],
                device_id=px, device_id_type=_MESH)
            part.start()
            parts.append(part)

        y_raw.wait_send()
        y_back.wait_send()

        @pl.when(mx == 1)
        def _():
            x_raw.wait_send()

        for part in parts:
            part.wait_send()
        mine = sbuf[...]
        for part in parts:
            part.wait_recv()
        o_ref[...] = mine + rbuf[...]

    f32 = jnp.float32
    return pl.pallas_call(
        body,
        out_shape=jax.ShapeDtypeStruct((1, n), x.dtype),
        in_specs=[pl.BlockSpec(memory_space=pl.ANY)],
        out_specs=pl.BlockSpec(memory_space=pltpu.VMEM),
        scratch_shapes=[
            pltpu.VMEM((m, n), f32),
            pltpu.VMEM((_RX, n), f32),
            pltpu.VMEM((_RY, n), f32),
            pltpu.VMEM((1, n), f32),
            pltpu.VMEM((1, n), f32),
            pltpu.VMEM((1, n), f32),
            pltpu.VMEM((1, n), f32),
            pltpu.SemaphoreType.DMA((len(chunks),)),
            pltpu.SemaphoreType.DMA((ncol,)),
            pltpu.SemaphoreType.DMA((ncol,)),
            pltpu.SemaphoreType.DMA((ncol,)),
            pltpu.SemaphoreType.DMA((3,)),
            pltpu.SemaphoreType.DMA((4,)),
            pltpu.SemaphoreType.REGULAR,
        ],
        compiler_params=pltpu.CompilerParams(
            collective_id=0,
            disable_bounds_checks=True,
            disable_semaphore_checks=True,
        ),
    )(x)
```

```python
import jax
import jax.numpy as jnp
from jax import lax
from jax.experimental import pallas as pl
from jax.experimental.pallas import tpu as pltpu

_MESH = pl.DeviceIdType.MESH

_RX = 112
_RY = 72
_MIDS = (96, 32)
_TAIL = 40
_LANES = 128

_NO_CHECKS = {
    name: True
    for name in ("disable_bounds_checks", "disable_semaphore_checks")
    if hasattr(pltpu.CompilerParams, name)
}


def _colsum8(ref, r0, nr, acc, blk=256):
    n = ref.shape[-1]
    r, end = r0, r0 + nr
    while r < end:
        b = min(blk, end - r)
        v = ref[pl.ds(r, b), :].reshape(b // 8, 8, n).sum(0)
        acc = v if acc is None else acc + v
        r += b
    return acc


def _sum_tiles(vals):
    a, b = vals[0], vals[1]
    for i, v in enumerate(vals[2:]):
        if i % 2 == 0:
            a = a + v
        else:
            b = b + v
    v = a + b
    v = v + pltpu.roll(v, 4, 0)
    v = (v + pltpu.roll(v, 1, 0)) + (pltpu.roll(v, 2, 0) + pltpu.roll(v, 3, 0))
    return v[0:1, :]


def pallas_dist_sum_ax0_xy_m2048_n1024_kernel(
x: jax.Array,
):
    m, n = x.shape
    first = _RX + _RY
    chunks = (m - first - sum(_MIDS) - _TAIL,) + _MIDS
    tail0 = m - _TAIL
    ncol = n // _LANES

    def body(x_hbm, o_ref, buf, xraw, yraw, ysend, yres, sbuf, rbuf,
             csem, tsem, ssem, rsem, xsem, ysem, yready):
        chunk_cps = []
        r0 = first
        for c, nr in enumerate(chunks):
            rows = pl.ds(r0, nr)
            cp = pltpu.make_async_copy(x_hbm.at[rows], buf.at[rows], csem.at[c])
            cp.start()
            chunk_cps.append((cp, r0, nr))
            r0 += nr
        tail_cps = []
        for c in range(ncol):
            blk = (pl.ds(tail0, _TAIL), pl.ds(c * _LANES, _LANES))
            cp = pltpu.make_async_copy(x_hbm.at[blk], buf.at[blk], tsem.at[c])
            cp.start()
            tail_cps.append(cp)

        mx = lax.axis_index("x")
        my = lax.axis_index("y")
        px = (1 - mx, my)
        py = (mx, 1 - my)

        x_own = pltpu.make_async_copy(
            x_hbm.at[pl.ds(0, _RX)], buf.at[pl.ds(0, _RX)], xsem.at[2])
        x_raw = pltpu.make_async_remote_copy(
            x_hbm.at[pl.ds(0, _RX)], xraw, xsem.at[0], xsem.at[1],
            device_id=px, device_id_type=_MESH)
        y_raw = pltpu.make_async_remote_copy(
            x_hbm.at[pl.ds(_RX, _RY)], yraw, ysem.at[0], ysem.at[1],
            device_id=py, device_id_type=_MESH)
        y_back = pltpu.make_async_remote_copy(
            ysend, yres, ysem.at[2], ysem.at[3],
            device_id=py, device_id_type=_MESH)

        barrier = pltpu.get_barrier_semaphore()
        pl.semaphore_signal(barrier, 1, device_id=px, device_id_type=_MESH)

        @pl.when(mx == 0)
        def _():
            x_own.start()

        @pl.when(my == 0)
        def _():
            pl.semaphore_signal(barrier, 1, device_id=py, device_id_type=_MESH)
            pl.semaphore_wait(barrier, 1)

        @pl.when(my == 1)
        def _():
            pl.semaphore_wait(barrier, 2)
            pl.semaphore_signal(yready, 1, device_id=py, device_id_type=_MESH)

        @pl.when(mx == 1)
        def _():
            x_raw.start()

        @pl.when(my == 0)
        def _():
            pl.semaphore_wait(yready, 1)

        y_raw.start()

        y_raw.wait_recv()
        ysend[...] = _colsum8(yraw, 0, _RY, None).sum(0, keepdims=True)
        y_back.start()

        cp, r0, nr = chunk_cps[0]
        cp.wait()
        acc = _colsum8(buf, r0, nr, None)

        def add_x_rows(acc):
            x_own.wait()
            acc = _colsum8(buf, 0, _RX, acc)
            x_raw.wait_recv()
            return _colsum8(xraw, 0, _RX, acc)

        acc = lax.cond(mx == 0, add_x_rows, lambda acc: acc, acc)

        y_back.wait_recv()
        row = lax.broadcasted_iota(jnp.int32, (8, n), 0)
        acc = acc + jnp.where(row == 0, jnp.broadcast_to(yres[...], (8, n)), 0.0)

        for cp, r0, nr in chunk_cps[1:]:
            cp.wait()
            acc = _colsum8(buf, r0, nr, acc)

        parts = []
        for c in range(ncol):
            cols = pl.ds(c * _LANES, _LANES)
            tail_cps[c].wait()
            sbuf[:, cols] = _sum_tiles(
                [acc[:, c * _LANES:(c + 1) * _LANES]]
                + [buf[pl.ds(tail0 + 8 * i, 8), cols] for i in range(_TAIL // 8)])
            part = pltpu.make_async_remote_copy(
                sbuf.at[:, cols], rbuf.at[:, cols], ssem.at[c], rsem.at[c],
                device_id=px, device_id_type=_MESH)
            part.start()
            parts.append(part)

        y_raw.wait_send()
        y_back.wait_send()

        @pl.when(mx == 1)
        def _():
            x_raw.wait_send()

        for part in parts:
            part.wait_send()
        mine = sbuf[...]
        for part in parts:
            part.wait_recv()
        o_ref[...] = mine + rbuf[...]

    f32 = jnp.float32
    return pl.pallas_call(
        body,
        out_shape=jax.ShapeDtypeStruct((1, n), x.dtype),
        in_specs=[pl.BlockSpec(memory_space=pl.ANY)],
        out_specs=pl.BlockSpec(memory_space=pltpu.VMEM),
        scratch_shapes=[
            pltpu.VMEM((m, n), f32),
            pltpu.VMEM((_RX, n), f32),
            pltpu.VMEM((_RY, n), f32),
            pltpu.VMEM((1, n), f32),
            pltpu.VMEM((1, n), f32),
            pltpu.VMEM((1, n), f32),
            pltpu.VMEM((1, n), f32),
            pltpu.SemaphoreType.DMA((len(chunks),)),
            pltpu.SemaphoreType.DMA((ncol,)),
            pltpu.SemaphoreType.DMA((ncol,)),
            pltpu.SemaphoreType.DMA((ncol,)),
            pltpu.SemaphoreType.DMA((3,)),
            pltpu.SemaphoreType.DMA((4,)),
            pltpu.SemaphoreType.REGULAR,
        ],
        compiler_params=pltpu.CompilerParams(collective_id=0, **_NO_CHECKS),
    )(x)
```
